```python
import numpy as np

kernel_name = "dist_sparse_attn_localglobal_htp_kvseq_b2_sq256_skv256_hq4_dh64"

def setup_inputs():
    x = np.random.randn(2, 256, 512).astype(np.float32)
    Wq = np.random.randn(512, 1024).astype(np.float32) * 0.02
    K_ext = np.random.randn(2, 1024, 16, 64).astype(np.float32)
    V_ext = np.random.randn(2, 1024, 16, 64).astype(np.float32)
    Wo = np.random.randn(1024, 512).astype(np.float32) * 0.02
    return {"x": x, "Wq": Wq, "K_ext": K_ext, "V_ext": V_ext, "Wo": Wo}

def reference(x, Wq, K_ext, V_ext, Wo):
    B, Sq, Skv, Hq, Dh = 2, 256, 1024, 16, 64
    Q = (x @ Wq).reshape(B, Sq, Hq, Dh)
    qi = np.arange(Sq)[:, None]
    ki = np.arange(Skv)[None, :]
    local = np.abs(qi - ki) <= 128
    glob = (ki < 32) | (qi < 32)
    mask = local | glob
    scores = np.einsum('bihd,bjhd->bhij', Q, K_ext).astype(np.float32) * 0.125
    scores = np.where(mask[None, None, :, :], scores, -1e9)
    scores_max = scores.max(axis=-1, keepdims=True)
    w = np.exp(scores - scores_max)
    row_keep = mask.any(axis=1)
    w_sum = np.where(row_keep[None, None, :, None], w.sum(axis=-1, keepdims=True), 1.0)
    w = w / w_sum
    w = np.where(row_keep[None, None, :, None], w, 0.0)
    ctx = np.einsum('bhij,bjhd->bihd', w, V_ext).reshape(B, Sq, Hq * Dh)
    return ctx @ Wo
```

```python
import jax
import jax.numpy as jnp
from jax import lax
from jax.experimental import pallas as pl
from jax.experimental.pallas import tpu as pltpu

bf, f32, u32 = jnp.bfloat16, jnp.float32, jnp.uint32
NEG = -1e30
QSCALE = 0.125 * 1.4426950408889634
MESH = pl.DeviceIdType.MESH

ROW_GROUPS = {'B0': (96, 0, 32), 'A0': (128, 1, 0), 'B1': (96, 2, 32), 'A1': (128, 3, 0), 'G': (64, 4, 0)}
N_PIECES = 8
GROUPABLE = ('cwq', 'prep', 'q', 'gq', 'at', 'aw', 'qx', 'g')


def allreduce_patterns():
    out = {}
    for keys, (a, b, c, d) in (('1CD', (0, 1, 2, 3)), ('3EF', (0, 3, 2, 1)), ('aGH', (1, 0, 3, 2)), ('bIJ', (3, 0, 1, 2))):
        fwd = ((a, b, -1), (b, c, 0), (c, d, 1))
        rev = ((d, c, -1), (c, b, 0), (b, a, 1))
        shift = lambda ms: tuple((x, y, p + 3 if p >= 0 else p) for x, y, p in ms)
        out[keys[0]] = fwd + shift(rev)
        out[keys[1]] = fwd + shift(rev[:2]) + ((d, a, 2),)
        out[keys[2]] = rev + shift(fwd[:2]) + ((a, d, 2),)
    return out


def build_tasks(cfg):
    tasks, have = [], {}

    def add(name, kind, chip, op, args, deps=(), dst=None):
        tasks.append(dict(name=name, kind=kind, chip=chip, op=op, args=args, deps=list(deps), dst=dst))
        return name

    def send(item, a, b):
        have[(item, b)] = add(f"{'.'.join(map(str, item))}:{a}{b}", 's', a, 'send', item, [have[(item, a)]], b)
        return have[(item, b)]

    def ship(item, a, b, via=None):
        if (item, b) in have:
            return have[(item, b)]
        if (a - b) % 4 == 2:
            via = via or (2 if a % 2 else 3)
            ship(item, a, via)
            a = via
        return send(item, a, b)

    home, wo = cfg['home'], {}
    pairs_at = {c: [p for p in range(8) if home[p] == c] for c in range(4)}
    for c in range(4):
        for p in (2 * c, 2 * c + 1):
            whole = None if p in cfg['wq_to_0'] else add(f'LWQ{p}', 'h', c, 'lwq', (p, None))
            for k in range(4):
                ld = whole or add(f'LWQ{p}.{k}', 'h', c, 'lwq', (p, k))
                have[(('W', p, k), c)] = add(f'CW{p}.{k}', 'c', c, 'cwq', (p, k), [ld])
                if p in cfg['wq_to_0']:
                    ship(('W', p, k), c, 0)
            whole = add(f'CO{p}', 'c', c, 'cwo', (p, None), [add(f'LWO{p}', 'h', c, 'lwo', (p, None))]) if home[p] == c else None
            for k in range(4):
                have[(('O', p, k), c)] = whole or add(f'CO{p}.{k}', 'c', c, 'cwo', (p, k), [add(f'LWO{p}.{k}', 'h', c, 'lwo', (p, k))])
            wo[p] = sorted({ship(('O', p, k), c, home[p]) for k in range(4)})
        if c in cfg['gq_direct']:
            add(f'LXG{c}', 'h', c, 'lxg', ())
        for n in range(4):
            add(f'CX{c}.{n}', 'c', c, 'cx', (n,), [add(f'LX{c}.{n}', 'h', c, 'lx', (n,))])
    for b in range(2):
        blocks = [(f'K0.{b}.{p}', 0, (b, p, 1, None)) for p in range(8)]
        for o in range(4):
            blocks += [(f'H{b}.{o}', 1, (b, 2 * o, 2, 0)), (f'K1.{b}.{o}', 1, (b, 2 * o, 2, 1))]
            blocks += [(f'K{c}.{b}.{o}', c, (b, 2 * o, 2, None)) for c in (2, 3)]
        for nm, c, args in blocks:
            add('P' + nm, 'c', c, 'prep', args, [add('L' + nm, 'h', c, 'lkv', args)])

    def get_q(p, n, c, via=None):
        it = ('Q', p, n)
        if (it, c) not in have:
            if (('W', p, 0), c) in have:
                deps = [have[(('W', p, k), c)] for k in range(4)] + [f'CX{c}.{n}']
                have[(it, c)] = add(f'Q{p}.{n}@{c}', 'c', c, 'q', (p, n), deps)
            else:
                get_q(p, n, p // 2)
                ship(it, p // 2, c, via)
        return have[(it, c)]

    for n in range(4):
        b, upper = n // 2, n % 2
        deps, src = {c: [] for c in range(4)}, {}
        for p in range(8):
            o, t = p // 2, home[p]
            window = [(x, p, b) for x in ('HK', 'HV')]
            for it in window:
                have.setdefault((it, 1), f'PH{b}.{o}')
            src[p] = 'CD' if upper else 'C'
            if (p, b) in cfg['kv0_to_home']:
                items = [(x, p, b, j) for x in 'KV' for j in range(2)]
                for it in items:
                    have.setdefault((it, 0), f'PK0.{b}.{p}')
                kv = [ship(it, 0, t, cfg['kv0_to_home'][(p, b)]) for it in items]
                have[(('C', p, n), t)] = add(f'AT{p}.{n}', 'c', t, 'at', (p, n, False), [get_q(p, n, t)] + kv)
            elif upper and (p, b) in cfg['kv1_to_0']:
                kv = [ship(it, 1, 0) for it in window] + [f'PK0.{b}.{p}']
                q0 = get_q(p, n, 0, cfg['q_via'].get((p, n)))
                have[(('N', p, n), 0)] = add(f'AT{p}.{n}', 'c', 0, 'at', (p, n, True), [q0] + kv)
                deps[t].append(ship(('N', p, n), 0, t))
                src[p] = 'C'
                continue
            else:
                q0 = get_q(p, n, 0, cfg['q_via'].get((p, n)))
                have[(('C', p, n), 0)] = add(f'AT{p}.{n}', 'c', 0, 'at', (p, n, False), [q0, f'PK0.{b}.{p}'])
            if upper and (p, b) in cfg['kv1_to_home']:
                kv = [ship(it, 1, t) for it in window]
                deps[t].append(add(f'AW{p}.{n}', 'c', t, 'aw', (p, n, False), [get_q(p, n, t)] + kv))
            elif upper:
                have[(('D', p, n), 1)] = add(f'AW{p}.{n}', 'c', 1, 'aw', (p, n, False), [get_q(p, n, 1), f'PH{b}.{o}'])
                deps[t].append(ship(('D', p, n), 1, t))
            deps[t].append(ship(('C', p, n), 0, t))
        rg = 'BA'[upper] + str(b)
        for c, ps in pairs_at.items():
            add(f'P{rg}@{c}', 'c', c, 'proj', (rg, n, tuple((p, src[p]) for p in ps)), deps[c] + [x for p in ps for x in wo[p]])

    deps, src = {c: [] for c in range(4)}, {}
    for p in range(8):
        o, t, it = p // 2, home[p], ('G', p)
        if o in cfg['gq_direct']:
            have[(it, o)] = add(f'GQ{p}', 'c', o, 'gq', (p,), [have[(('W', p, k), o)] for k in range(4)] + [f'LXG{o}'])
        else:
            get_q(p, 0, o), get_q(p, 2, o)
        for c in range(4):
            if (c != 0 or o == 0) and (it, c) not in have and all((('Q', p, n), c) in have for n in (0, 2)):
                have[(it, c)] = add(f'QX{p}@{c}', 'c', c, 'qx', (p,), [have[(('Q', p, n), c)] for n in (0, 2)])
        for a, bb in (cfg['g0_hops'][p] if o == 0 else ((o, 2), (2, 1), (2, 3))):
            ship(it, a, bb)
        for c in (1, 2, 3):
            keys = [f'PK{c}.{b}.{o}' for b in range(2)] + ([f'PH{b}.{o}' for b in range(2)] if c == 1 else [])
            have[(('E', p, c), c)] = add(f'GL{p}@{c}', 'c', c, 'g', (p, c), [have[(it, c)]] + keys)
        chains = cfg['e0_chains'][p] if t == 0 else {1: ((3, 2, 1),), 2: ((1, 2), (3, 2)), 3: ((1, 2, 3),)}[t]
        for seq in chains:
            for i in range(len(seq) - 1):
                a = seq[i]
                if i:
                    both = [have[(('E', p, seq[i - 1]), a)], have[(('E', p, a), a)]]
                    have[(('E', p, a), a)] = add(f'GM{p}@{a}', 'c', a, 'gm', (p, a, seq[i - 1]), both)
                send(('E', p, a), a, seq[i + 1])
        src[p] = tuple(seq[-2] for seq in chains) + ((t,) if t else ())
        deps[t] += [have[(('E', p, x), t)] for x in src[p]] + [have[(('C', p, n), t)] for n in (0, 2)] + wo[p]
    for c, ps in pairs_at.items():
        add(f'PG@{c}', 'c', c, 'projg', tuple((p, src[p]) for p in ps), deps[c])

    patterns = allreduce_patterns()
    for g, (rg, (rows, _, _)) in enumerate(ROW_GROUPS.items()):
        for j, key in enumerate(cfg['allreduce'][rg]):
            geo = (rg, g * N_PIECES + j, 128 * (j // 2), rows // 2 * (j % 2), rows // 2)
            msgs, names, terms = patterns[key], [f'R{rg}.{j}.{i}' for i in range(6)], []
            rslot = [sum(m[1] == msgs[i][1] for m in msgs[:i]) for i in range(6)]
            for i, (a, bb, prev) in enumerate(msgs):
                terms.append(1 + (terms[prev] if prev >= 0 else 0))
                item = ('R', geo, sum(m[0] == a for m in msgs[:i]), rslot[i], rslot[prev] if prev >= 0 else None)
                add(names[i], 's', a, 's3', item, [f'P{rg}@{a}'] + ([names[prev]] if prev >= 0 else []), bb)
            for c in range(4):
                got = [i for i in range(6) if msgs[i][1] == c]
                own = terms[got[-1]] < 4
                add(f'F{rg}.{j}@{c}', 'c', c, 'fin', (geo, own, tuple(rslot[i] for i in got)),
                    ([f'P{rg}@{c}'] if own else []) + [names[i] for i in got])
    return tasks


def unpack(x):
    return pltpu.bitcast(x, bf)


def pack(x):
    return pltpu.bitcast(x.astype(bf), u32)


def dot(a, b):
    return jnp.dot(a, b, preferred_element_type=f32)


def dot_nt(a, b):
    return lax.dot_general(a, b, (((1,), (1,)), ((), ())), preferred_element_type=f32)


def lanes(rows):
    return lax.broadcasted_iota(jnp.int32, (rows, 128), 1)


def softmax_pv(scores, apply_v, store):
    probs = []
    for s in scores:
        m = s[0].max(axis=0, keepdims=True)
        for x in s[1:]:
            m = jnp.maximum(m, x.max(axis=0, keepdims=True))
        e = [jnp.exp2(x - m) for x in s]
        l = e[0].sum(axis=0, keepdims=True)
        for x in e[1:]:
            l = l + x.sum(axis=0, keepdims=True)
        probs.append(([x.astype(bf) for x in e], m, l))
    for (e, m, l), v, out in zip(probs, apply_v, store):
        out(v(e) * (1.0 / l), m + jnp.log2(l))


def merge(parts):
    m = parts[0][1]
    for _, l in parts[1:]:
        m = jnp.maximum(m, l)
    es = [jnp.exp2(l - m) for _, l in parts]
    tot = es[0]
    for e in es[1:]:
        tot = tot + e
    r = 1.0 / tot
    acc = parts[0][0] * (es[0] * r)
    for (c, _), e in zip(parts[1:], es[1:]):
        acc = acc + c * (e * r)
    return acc, m + jnp.log2(tot)


def compact(get):
    r = get(0, 0)
    for g in range(1, 4):
        t = pltpu.roll(get(g // 2, g % 2), 32 * g, 1)
        r = jnp.where(lanes(t.shape[0]) >= 32 * g, t, r)
    return r


def make_kernel(cfg, programs):
    tasks = build_tasks(cfg)
    by_name = {t['name']: t for t in tasks}
    assert len(by_name) == len(tasks)
    lidx, sidx, ridx = {}, {}, {}
    for c in range(4):
        lidx.update({t['name']: 2 * i for i, t in enumerate(t for t in tasks if t['kind'] == 'h' and t['chip'] == c)})
        sidx.update({t['name']: i for i, t in enumerate(t for t in tasks if t['kind'] == 's' and t['chip'] == c)})
        ridx.update({t['name']: i for i, t in enumerate(t for t in tasks if t['kind'] == 's' and t['dst'] == c)})

    def body(x_hbm, wq_hbm, k_hbm, v_hbm, wo_hbm, o_ref, xg, xf, xb, wqf, wqt, wof, wob, kf, vf, kb, vb,
             kx, vx, hk, hv, qb, cb, db, gb, eb, bias, pb, sb, rb, lsem, ssem, rsem, ready):
        me = lax.axis_index("i")
        barrier = pltpu.get_barrier_semaphore()

        def remote(t):
            it, a = t['args'], t['chip']
            k = it[0]
            if k == 'K':
                sl = (it[2], it[1], pl.ds(64 * it[3], 64))
                src, dst = (kb if a == 0 else kx).at[sl], kx.at[sl]
            elif k == 'V':
                sl = (it[2], it[1], pl.ds(32 * it[3], 32))
                src, dst = (vb if a == 0 else vx).at[sl], vx.at[sl]
            elif k == 'HK':
                dst = hk.at[it[2], it[1]]
                src = kb.at[it[2], it[1], pl.ds(0, 64)] if a == 1 else dst
            elif k == 'HV':
                dst = hv.at[it[2], it[1]]
                src = vb.at[it[2], it[1], :, pl.ds(0, 128)] if a == 1 else dst
            elif k == 'R':
                rows = pl.ds(0, it[1][4] // 2)
                src, dst = sb.at[it[1][1], it[2], rows], rb.at[it[1][1], it[3], rows]
            elif k == 'N':
                src = dst = cb.at[it[1], it[2], pl.ds(0, 64)]
            elif k == 'O':
                src = dst = wob.at[it[1], :, pl.ds(128 * it[2], 128)]
            elif k == 'D':
                src = dst = db.at[it[1], it[2] // 2]
            elif k == 'G':
                src = dst = gb.at[it[1]]
            else:
                src = dst = {'W': wqt, 'Q': qb, 'C': cb, 'E': eb}[k].at[it[1], it[2]]
            return pltpu.make_async_remote_copy(src, dst, ssem.at[sidx[t['name']]], rsem.at[ridx[t['name']]],
                                                device_id=(t['dst'],), device_id_type=MESH)

        def local(t):
            op, a, i = t['op'], t['args'], lidx[t['name']]
            if op == 'lx':
                pairs = [(x_hbm.at[a[0]], xf.at[a[0]])]
            elif op == 'lxg':
                pairs = [(x_hbm.at[2 * b, pl.ds(0, 32)], xg.at[pl.ds(32 * b, 32)]) for b in range(2)]
            elif op == 'lwq':
                rows = pl.ds(0, 512) if a[1] is None else pl.ds(128 * a[1], 128)
                pairs = [(wq_hbm.at[rows, pl.ds(128 * (a[0] % 2), 128)], wqf.at[a[0] % 2, rows])]
            elif op == 'lwo':
                cols = pl.ds(0, 512) if a[1] is None else pl.ds(128 * a[1], 128)
                pairs = [(wo_hbm.at[pl.ds(128 * (a[0] % 2), 128), cols], wof.at[a[0] % 2, :, cols])]
            else:
                b, p, k, h = a
                sl = (b, pl.ds(p, k)) if h is None else (b, pl.ds(p, k), slice(None), pl.ds(128 * h, 128))
                pairs = [(k_hbm.at[sl], kf.at[sl]), (v_hbm.at[sl], vf.at[sl])]
            return [pltpu.make_async_copy(s, d, lsem.at[i + j]) for j, (s, d) in enumerate(pairs)]

        def attention(ts, chip0_keys, c):
            zero = jnp.zeros((64, 128), bf)
            scores, apply_v, store = [], [], []
            for t in ts:
                p, n, both = t['args']
                b = n // 2
                masks = ([1, None] if n % 2 else [None, 0]) if chip0_keys else [2]
                dst = cb.at[p, n] if chip0_keys else db.at[p, b]
                kk, vv = (kb, vb) if c == (0 if chip0_keys else 1) else ((kx, vx) if chip0_keys else (hk, hv))
                for h in range(2):
                    qt = unpack(qb[p, n, 32 * h:32 * h + 32, :])
                    w = jnp.concatenate([zero, qt] if h else [qt, zero], 0)
                    s = [dot(unpack(kk[b, p, 64 * j:64 * j + 64, :]), w) for j in range(len(masks))]
                    s = [x if k is None else x + bias[k] for x, k in zip(s, masks)]
                    scores.append(s + [dot(unpack(hk[b, p]), w) + bias[2]] if both else s)

                    def pv(e, p=p, b=b, h=h, vv=vv):
                        o = dot(unpack(vv[b, p, 32 * h:32 * h + 32, 0:128]), e[0])
                        if len(e) > 1:
                            o = o + dot(unpack(vv[b, p, 32 * h:32 * h + 32, 128:256]), e[1])
                        if len(e) > 2:
                            o = o + dot(unpack(hv[b, p, 32 * h:32 * h + 32, :]), e[2])
                        return o

                    def out(o, lse, dst=dst, h=h):
                        dst[32 * h:32 * h + 32, :] = pack(o)
                        dst[64 + h:65 + h, :] = pltpu.bitcast(lse, u32)

                    apply_v.append(pv)
                    store.append(out)
            softmax_pv(scores, apply_v, store)

        def store_e(p, c, o, lse):
            eb[p, c, 0:32, :] = pack(o)
            eb[p, c, 32:33, :] = pltpu.bitcast(lse, u32)

        def global_attention(ts):
            grp = lanes(64) // 32
            scores, apply_v, store = [], [], []
            for t in ts:
                p, c = t['args']
                g = unpack(gb[p])
                z = jnp.zeros_like(g)
                ws = [jnp.concatenate([jnp.where(grp == b, g, z), jnp.where(grp == 2 + b, g, z)], 0) for b in range(2)]
                scores.append([dot(unpack(kb[0, p, 64 * j:64 * j + 64, :]), ws[0])
                               + dot(unpack(kb[1, p, 64 * j:64 * j + 64, :]), ws[1]) for j in range(2)])

                def pv(e, p=p):
                    e = jnp.concatenate(e, 0)
                    o0, o1 = dot(unpack(vb[0, p]), e), dot(unpack(vb[1, p]), e)
                    return jnp.where(grp == 0, o0[:64], jnp.where(grp == 1, o1[:64], jnp.where(grp == 2, o0[64:], o1[64:])))

                apply_v.append(pv)
                store.append(lambda o, lse, p=p, c=c: store_e(p, c, o, lse))
            softmax_pv(scores, apply_v, store)

        def head_ctx(ref, h):
            return unpack(ref[32 * h:32 * h + 32, :]).astype(f32)

        def head_lse(ref, h):
            return pltpu.bitcast(ref[64 + h:65 + h, :], f32)

        def merged(p, n):
            refs = (cb.at[p, n], db.at[p, n // 2])
            return jnp.concatenate([merge([(head_ctx(r, h), head_lse(r, h)) for r in refs])[0] for h in range(2)], 0)

        def e_part(p, c):
            return unpack(eb[p, c, 0:32, :]).astype(f32), pltpu.bitcast(eb[p, c, 32:33, :], f32)

        def own_piece(geo):
            rg, _, c0, r0, nr = geo
            r0 += ROW_GROUPS[rg][2]
            return pb[ROW_GROUPS[rg][1], r0:r0 + nr, c0:c0 + 128]

        def received(geo, slot):
            return unpack(rb[geo[1], slot, 0:geo[4] // 2, :]).astype(f32)

        def wq_rows(ts):
            return jnp.concatenate(
                [jnp.concatenate([unpack(wqt[t['args'][0], k]) for k in range(4)], 1) for t in ts], 0)

        def project(cols, pairs):
            return dot(jnp.concatenate(cols, 1), jnp.concatenate([unpack(wob[p]) for p, _ in pairs], 0))

        def compute(ts, c):
            op, a = ts[0]['op'], ts[0]['args']
            if op == 'cwq':
                for t in ts:
                    p, k = t['args']
                    wqt[p, k] = pack((wqf[p % 2, 128 * k:128 * k + 128, :] * QSCALE).astype(bf).T)
            elif op == 'cx':
                xb[a[0]] = pack(xf[a[0]])
            elif op == 'cwo':
                cols = slice(0, 512) if a[1] is None else slice(128 * a[1], 128 * a[1] + 128)
                wob[a[0], :, cols] = pack(wof[a[0] % 2, :, cols])
            elif op == 'prep':
                for t in ts:
                    b, p0, k, h = t['args']
                    k0, nk = (0, 256) if h is None else (128 * h, 128)
                    for p in range(p0, p0 + k):
                        kb[b, p, k0 // 2:(k0 + nk) // 2, :] = pack(kf[b, p, :, k0:k0 + nk].astype(bf).T)
                        vb[b, p, :, k0:k0 + nk] = pack(vf[b, p, :, k0:k0 + nk])
            elif op == 'q':
                q = dot_nt(wq_rows(ts), unpack(xb[a[1]]))
                for i, t in enumerate(ts):
                    qb[t['args'][0], a[1]] = pack(q[128 * i:128 * i + 128])
            elif op == 'gq':
                xx = xg[...].astype(bf)
                q = dot_nt(wq_rows(ts), jnp.concatenate([xx, xx], 0))
                for i, t in enumerate(ts):
                    gb[t['args'][0]] = pack(jnp.where(lanes(64) < 64, q[128 * i:128 * i + 64], q[128 * i + 64:128 * i + 128]))
            elif op in ('at', 'aw'):
                attention(ts, op == 'at', c)
            elif op == 'proj':
                rg, n, pairs = a
                cols = [(unpack(cb[p, n, 0:64, :]) if s == 'C' else merged(p, n).astype(bf)).T for p, s in pairs]
                pb[ROW_GROUPS[rg][1]] = project(cols, pairs)
            elif op == 'qx':
                for t in ts:
                    p = t['args'][0]
                    gb[p] = pack(compact(lambda h, b: head_ctx(qb.at[p, 2 * b], h)))
            elif op == 'g':
                global_attention(ts)
            elif op == 'gm':
                store_e(a[0], a[1], *merge([e_part(a[0], a[1]), e_part(a[0], a[2])]))
            elif op == 'projg':
                cols = []
                for p, srcs in a:
                    part0 = (compact(lambda h, b: head_ctx(cb.at[p, 2 * b], h)),
                             compact(lambda h, b: head_lse(cb.at[p, 2 * b], h)))
                    m, _ = merge([part0] + [e_part(p, s) for s in srcs])
                    cols.append(jnp.concatenate([m, pltpu.roll(m, 64, 1)], 0).astype(bf).T[0:64])
                pb[4, 0:64, :] = project(cols, a)
            elif op == 's3':
                _, geo, sslot, _, prev = a
                v = own_piece(geo) if prev is None else own_piece(geo) + received(geo, prev)
                sb[geo[1], sslot, 0:geo[4] // 2, :] = pack(v)
            elif op == 'fin':
                geo, own, slots = a
                rg, _, c0, r0, nr = geo
                vals = ([own_piece(geo)] if own else []) + [received(geo, s) for s in slots]
                v = vals[0]
                for u in vals[1:]:
                    v = v + u
                b, r0 = (r0 // 32, 0) if rg == 'G' else (int(rg[1]), r0 + (128 if rg[0] == 'A' else 32))
                o_ref[b, r0:r0 + nr, c0:c0 + 128] = v
            else:
                raise ValueError(op)

        def notify(sem, d):
            pl.semaphore_signal(sem, inc=1, device_id=(d,), device_id_type=MESH)

        def leading_loads(c):
            n = 0
            while by_name[programs[c][n]]['kind'] == 'h':
                n += 1
            return n

        def prologue(c):
            if c != 2:
                notify(barrier, (c + 1) % 4)
                notify(barrier, (c + 3) % 4)
            for name in programs[c][:leading_loads(c)]:
                for cp in local(by_name[name]):
                    cp.start()
            if c in (1, 3):
                pl.semaphore_wait(barrier, 1)
            if c == 2:
                pl.semaphore_wait(barrier, 2)
                notify(ready, 1)
                notify(ready, 3)

        def run(c):
            prog = programs[c]
            done, sending, loading = set(), set(), set(prog[:leading_loads(c)])
            handshake = {d: None for d in range(4)}
            if c == 0:
                handshake = {1: (barrier, 2), 3: (barrier, 2)}
            elif c != 2:
                handshake[2] = (ready, 1)

            def need(dep):
                t = by_name[dep]
                if dep in done:
                    return
                assert t['kind'] != 'c', dep
                done.add(dep)
                if t['kind'] == 'h':
                    assert dep in loading, dep
                    for cp in local(t):
                        cp.wait()
                else:
                    remote(t).wait_recv()

            ops = {t['op'] for t in tasks if t['chip'] == c}
            ki = lax.broadcasted_iota(jnp.int32, (128, 128), 0)
            qi = lanes(128)
            if 'at' in ops:
                bias[0] = jnp.where((ki <= qi) | (qi < 32), 0.0, NEG).astype(f32)
                bias[1] = jnp.where((ki >= qi) | (ki < 32), 0.0, NEG).astype(f32)
            if 'aw' in ops or c == 0:
                bias[2] = jnp.where(ki <= qi, 0.0, NEG).astype(f32)

            i = leading_loads(c)
            while i < len(prog):
                name = prog[i]
                i += 1
                if name.startswith('WS:'):
                    sending.remove(name[3:])
                    remote(by_name[name[3:]]).wait_send()
                    continue
                t = by_name[name]
                if t['kind'] == 'h':
                    loading.add(name)
                    for cp in local(t):
                        cp.start()
                    continue
                group = [t]
                while t['op'] in GROUPABLE and len(group) < 4 and i < len(prog):
                    u = by_name.get(prog[i])
                    if u is None or u['op'] != t['op'] or (t['op'] == 'q' and u['args'][1] != t['args'][1]):
                        break
                    group.append(u)
                    i += 1
                for u in group:
                    for d in u['deps']:
                        need(d)
                if t['op'] != 'send':
                    compute(group, c)
                if t['kind'] == 'c':
                    done.update(u['name'] for u in group)
                    continue
                if handshake[t['dst']]:
                    pl.semaphore_wait(*handshake[t['dst']])
                    handshake = {d: None for d in range(4)}
                remote(t).start()
                sending.add(name)
            assert not sending
            assert all(t['name'] in done for t in tasks if (t['dst'] if t['kind'] == 's' else t['chip']) == c)

        for c in range(4):
            pl.when(me == c)(lambda c=c: prologue(c))
        for c in (3, 1, 2, 0):
            pl.when(me == c)(lambda c=c: run(c))

    def kernel(x, Wq, K_ext, V_ext, Wo):
        kt = K_ext.transpose(0, 2, 3, 1).reshape(2, 8, 128, 256)
        vt = V_ext.transpose(0, 2, 3, 1).reshape(2, 8, 128, 256)
        v, sem = pltpu.VMEM, pltpu.SemaphoreType.DMA
        n_piece = N_PIECES * len(ROW_GROUPS)
        scratch = [
            v((64, 512), f32), v((4, 128, 512), f32), v((4, 64, 512), u32),
            v((2, 512, 128), f32), v((8, 4, 64, 128), u32),
            v((2, 128, 512), f32), v((8, 64, 512), u32),
            v((2, 8, 128, 256), f32), v((2, 8, 128, 256), f32),
            v((2, 8, 128, 128), u32), v((2, 8, 64, 256), u32),
            v((2, 8, 128, 128), u32), v((2, 8, 64, 256), u32),
            v((2, 8, 64, 128), u32), v((2, 8, 64, 128), u32),
            v((8, 4, 64, 128), u32), v((8, 4, 66, 128), u32), v((8, 2, 66, 128), u32),
            v((8, 32, 128), u32), v((8, 4, 33, 128), u32),
            v((3, 128, 128), f32), v((5, 128, 512), f32),
            v((n_piece, 2, 32, 128), u32), v((n_piece, 2, 32, 128), u32),
            sem((max(lidx.values()) + 2,)), sem((max(sidx.values()) + 1,)), sem((max(ridx.values()) + 1,)),
            pltpu.SemaphoreType.REGULAR,
        ]
        return pl.pallas_call(
            body,
            out_shape=jax.ShapeDtypeStruct((2, 256, 512), f32),
            in_specs=[pl.BlockSpec(memory_space=pl.ANY)] * 5,
            out_specs=pl.BlockSpec(memory_space=pltpu.VMEM),
            scratch_shapes=scratch,
            compiler_params=pltpu.CompilerParams(
                collective_id=0, vmem_limit_bytes=64 * 1024 * 1024, disable_semaphore_checks=True),
        )(x.reshape(4, 128, 512), Wq, kt, vt, Wo)

    return kernel


CONFIG = {'home': (0, 0, 1, 1, 1, 2, 3, 0),
 'wq_to_0': (3,),
 'kv0_to_home': {(2, 0): None, (5, 0): 3, (5, 1): 3},
 'kv1_to_home': ((6, 0), (6, 1)),
 'kv1_to_0': ((0, 1), (7, 0), (7, 1)),
 'gq_direct': (1, 2, 3),
 'q_via': {(4, 0): 3, (4, 1): 1, (4, 2): 3, (4, 3): 1},
 'g0_hops': {0: ((0, 1), (1, 2), (2, 3)), 1: ((0, 1), (1, 2), (2, 3))},
 'e0_chains': {0: ((1, 2, 3, 0),), 1: ((1, 2, 3, 0),), 7: ((1, 2, 3, 0),)},
 'allreduce': {'B0': '33J3333F', 'A0': 'E1311E1E', 'B1': 'I33E3b3D', 'A1': 'D3DD3Fba', 'G': 'DFF33FF3'}}

PROGRAMS = [
    (
        'LWQ0 LK0.0.2 LK0.1.5 LX0.2 LWQ1 LX0.1 LX0.0 LK0.0.5 LK0.1.0 CW0.1 LK0.1.6 LK0.1.1 PK0.1.5 PK0.0.2 '
        'LK0.0.6 V.2.0.1:01 K.2.0.0:01 K.5.1.0:03 K.2.0.1:01 V.2.0.0:01 LK0.0.3 CW1.1 CW1.0 CW0.2 CW0.3 '
        'V.5.1.1:03 LK0.1.3 CX0.1 CX0.2 CW1.2 CW1.3 CW0.0 LK0.1.2 V.5.1.0:03 CX0.0 K.5.1.1:03 Q1.0@0 Q1.1@0 '
        'LK0.0.4 PK0.0.5 LK0.1.7 Q0.1@0 Q0.2@0 Q1.2@0 LWO0 WS:V.2.0.1:01 WS:K.5.1.0:03 Q0.0@0 LX0.3 V.5.0.1:03 '
        'PK0.1.1 QX0@0 QX1@0 LK0.1.4 WS:K.2.0.0:01 WS:V.5.1.1:03 V.5.0.0:03 G.1:01 K.5.0.0:03 G.0:01 PK0.0.6 '
        'PK0.1.6 PK0.1.0 LK0.0.0 Q.0.1:01 AT0.2 AT6.0 LWO1 WS:K.2.0.1:01 WS:V.5.1.0:03 Q.1.1:01 PK0.0.3 PK0.1.3 '
        'LK0.0.7 Q3.0@0 LK0.0.1 WS:V.2.0.0:01 WS:K.5.1.1:03 Q3.2@0 AT6.2 AT3.0 WS:V.5.0.1:03 WS:G.1:01 WS:G.0:01 '
        'K.5.0.1:03 C.3.0:01 Q3.1@0 AT6.3 AT3.2 WS:V.5.0.0:03 WS:Q.0.1:01 C.6.3:03 CX0.3 C.3.2:01 PK0.1.2 PK0.1.4 '
        'PK0.0.4 PK0.1.7 AT4.2 AT4.0 WS:K.5.0.0:03 WS:Q.1.1:01 C.4.0:01 C.4.2:01 CO1 CO0 C.6.2:03 Q3.3@0 C.6.0:03 '
        'AT3.3 AT6.1 AT3.1 AT2.2 WS:K.5.0.1:03 WS:C.3.0:01 C.6.1:03 Q1.3@0 WS:C.6.3:03 WS:C.3.2:01 C.2.2:01 '
        'PK0.0.7 PK0.0.0 PK0.0.1 Q.1.3:01 AT1.2 AT2.3 AT7.2 AT0.0 WS:C.4.0:01 WS:C.6.2:03 PB1@0 RB1.1.0 '
        'WS:C.4.2:01 RB1.2.0 RB1.3.0 C.3.3:01 RB1.4.0 WS:C.6.0:03 C.2.3:01 RB1.6.0 AT1.0 AT4.3 AT7.0 WS:C.6.1:03 '
        'WS:C.2.2:01 PB0@0 RB0.6.0 RB0.1.0 C.4.3:01 C.3.1:01 RB0.5.0 RB0.4.0 RB0.3.0 AT7.1 AT1.3 AT1.1 AT0.1 '
        'WS:Q.1.3:01 WS:RB1.1.0 WS:RB1.2.0 WS:RB1.3.0 PA0@0 WS:C.3.3:01 WS:RB1.4.0 WS:RB1.6.0 RA0.0.0 RA0.2.0 '
        'RA0.7.0 AT4.1 WS:C.2.3:01 WS:RB0.6.0 RA0.5.0 C.4.1:01 RA0.4.0 WS:RB0.1.0 RA0.1.0 RB0.0.0 RB1.5.5 Q0.3@0 '
        'WS:RB0.5.0 RB1.0.1 FB1.5@0 AT0.3 AT7.3 WS:C.4.3:01 WS:RB0.4.0 WS:RB0.3.0 RA0.3.0 WS:RA0.0.0 RB0.7.3 '
        'RA0.6.0 RB0.2.4 PG@0 WS:C.3.1:01 WS:RA0.2.0 RG.7.0 RG.4.0 RG.3.0 RG.1.3 PA1@0 WS:RA0.7.0 WS:RA0.5.0 '
        'WS:C.4.1:01 FB0.4@0 FB1.0@0 RA1.1.0 RG.0.3 RA1.6.1 RG.5.3 RG.6.3 FB0.1@0 RA1.4.0 WS:RA0.4.0 WS:RA0.1.0 '
        'WS:RB0.0.0 WS:RB1.5.5 WS:RB1.0.1 WS:RB0.7.3 FB0.2@0 FB0.5@0 FB1.7@0 FB0.7@0 FA1.3@0 RA1.7.1 RB1.7.3 '
        'FB0.0@0 RB1.5.1 RA1.3.3 WS:RG.7.0 RA1.7.5 RA1.0.5 RB0.2.2 RB1.7.5 WS:RA0.3.0 WS:RA0.6.0 WS:RB0.2.4 '
        'WS:RG.4.0 WS:RG.3.0 WS:RG.1.3 FA1.0@0 FB0.6@0 FB1.1@0 FA1.7@0 FB1.2@0 RG.2.5 FA1.6@0 RA1.0.3 WS:RA1.1.0 '
        'RA1.2.3 RB0.7.5 RG.2.3 WS:RG.0.3 RA1.5.3 WS:RA1.6.1 WS:RG.5.3 WS:RG.6.3 WS:RA1.4.0 WS:RA1.7.1 WS:RB1.7.3 '
        'WS:RB1.5.1 FB1.6@0 FA0.6@0 FB1.4@0 FG.2@0 FA0.4@0 FG.1@0 FG.4@0 FA0.3@0 FG.7@0 RA1.2.5 WS:RA1.3.3 FG.5@0 '
        'RG.6.5 FA0.1@0 RA1.3.5 WS:RA1.0.5 RA1.6.5 RG.1.5 FG.3@0 RA1.5.5 RG.5.5 RG.0.5 WS:RA1.7.5 WS:RB0.2.2 '
        'WS:RG.2.5 WS:RB1.7.5 FA1.2@0 WS:RG.2.3 FA1.5@0 WS:RA1.0.3 FG.0@0 FG.6@0 WS:RA1.5.3 WS:RA1.2.3 FA0.0@0 '
        'FA1.1@0 WS:RB0.7.5 WS:RA1.2.5 FB1.3@0 WS:RG.6.5 FA1.4@0 WS:RG.1.5 WS:RA1.3.5 FA0.7@0 FB0.3@0 WS:RA1.5.5 '
        'WS:RA1.6.5 FA0.5@0 FA0.2@0 WS:RG.5.5 WS:RG.0.5'
    ).split(),
    (
        'LWQ3.0 LWQ3.1 LWQ2 LWQ3.2 LH1.3 LWQ3.3 LXG1 LX1.3 LX1.2 LX1.0 LK1.1.3 CW3.0 LH0.3 W.3.0:10 LH1.0 CW2.2 '
        'CW3.2 W.3.2:10 LH1.2 PH1.3 HK.6.1:12 CW2.1 CW3.3 CW2.3 CW2.0 CW3.1 LK1.0.0 LK1.1.0 W.3.1:10 CX1.3 '
        'W.3.3:10 HV.6.1:12 GQ2 LH0.0 Q2.3@1 HV.7.1:10 Q.2.3:10 G.2:12 LK1.0.3 WS:W.3.0:10 CX1.0 CX1.2 Q2.2@1 '
        'Q3.3@1 LH0.2 GQ3 LWO3 WS:W.3.2:10 G.3:12 PH0.3 WS:HK.6.1:12 HV.6.0:12 HV.7.0:10 PK1.1.3 LK1.0.2 Q2.0@1 '
        'LK1.1.1 WS:W.3.1:10 Q.2.2:10 PH1.0 WS:HV.6.1:12 HK.6.0:12 PH1.2 LH1.1 WS:G.2:12 AT2.0 LK1.1.2 '
        'WS:W.3.3:10 HK.0.1:10 PK1.0.0 PK1.1.0 LWO2 WS:G.3:12 Q.4.3:10 G.0:12 AW5.3 LH0.1 WS:HV.7.1:10 HK.7.1:10 '
        'G.1:12 D.5.3:12 PH0.0 PK1.0.3 LK1.0.1 WS:HV.6.0:12 GL0@1 GL6@1 GL7@1 GL1@1 LX1.1 WS:Q.2.3:10 '
        'WS:HK.6.0:12 E.1.1:12 PK1.0.2 PH0.2 WS:HV.7.0:10 WS:G.0:12 E.6.1:12 E.7.1:12 AW0.1 AW4.3 WS:G.1:12 '
        'E.0.1:12 AW5.1 WS:Q.2.2:10 D.5.1:12 PK1.1.2 WS:D.5.3:12 CO3 CO2 AW1.1 WS:HK.0.1:10 WS:E.1.1:12 HK.7.0:10 '
        'D.0.1:10 GL5@1 WS:E.6.1:12 E.5.1:12 PB0@1 WS:Q.4.3:10 WS:E.7.1:12 RB0.6.3 PH0.1 PH1.1 PK1.0.1 PK1.1.1 '
        'WS:HK.7.1:10 WS:E.0.1:12 RB0.4.3 RB0.5.3 RB0.1.3 RB0.0.3 D.1.1:10 CX1.1 RB0.7.0 Q.4.1:10 GL2@1 GL4@1 '
        'GL3@1 WS:D.5.1:12 WS:HK.7.0:10 PB1@1 WS:E.5.1:12 WS:RB0.6.3 RB1.5.4 RB1.6.3 RB1.1.3 RB1.2.3 AW2.3 AW1.3 '
        'AW3.3 AW4.1 WS:D.0.1:10 WS:RB0.4.3 WS:RB0.5.3 RB1.4.3 HV.0.1:10 D.1.3:10 PG@1 WS:RB0.1.3 WS:RB0.0.3 '
        'WS:D.1.1:10 RG.1.0 RG.2.0 RG.4.3 Q3.1@1 Q2.1@1 WS:RB0.7.0 RG.6.0 WS:RB1.6.3 RB1.0.4 WS:Q.4.1:10 RB0.2.1 '
        'RG.7.3 RG.3.3 RB1.3.3 WS:RB1.5.4 WS:RB1.1.3 RB1.7.2 RG.5.0 WS:RB1.2.3 PA1@1 WS:RB1.4.3 WS:HV.0.1:10 '
        'WS:RG.1.0 RA1.5.0 WS:RG.2.0 RA1.3.2 RA1.1.3 RA1.0.2 RA1.4.3 AW2.1 AW3.1 WS:RG.4.3 WS:RG.6.0 RA1.7.0 '
        'AT2.1 WS:D.1.3:10 WS:RB1.0.4 WS:RG.7.3 WS:RG.3.3 RA1.6.4 RB0.3.3 WS:RB1.3.3 PA0@1 WS:RB0.2.1 WS:RB1.7.2 '
        'WS:RG.5.0 RA0.2.3 RA0.6.5 RA0.4.5 RA0.0.3 WS:RA1.5.0 WS:RA1.3.2 RA0.1.1 RA0.3.5 WS:RA1.1.3 RB1.0.2 '
        'RA0.5.3 RA0.1.5 FA0.4@1 RA1.2.2 WS:RA1.0.2 RA0.7.3 WS:RA1.4.3 WS:RA1.7.0 WS:RB0.3.3 FB1.2@1 FA0.1@1 '
        'FB1.4@1 FB1.0@1 RA0.6.1 RG.0.2 WS:RA1.6.4 WS:RA0.2.3 WS:RA0.6.5 FB0.6@1 FA0.3@1 FB1.3@1 RA0.0.5 RA0.4.1 '
        'RB1.3.5 RA0.3.1 WS:RA0.4.5 WS:RA0.0.3 WS:RA0.1.1 WS:RA0.3.5 FA0.6@1 FB0.5@1 FB0.2@1 FG.0@1 FA0.0@1 '
        'RA0.7.5 RB1.7.4 RG.0.4 WS:RB1.0.2 RB1.5.2 WS:RA0.1.5 FB1.6@1 FA1.6@1 RA0.5.5 WS:RA0.5.3 FB1.7@1 RA1.3.4 '
        'RA1.6.2 WS:RA1.2.2 WS:RA0.7.3 WS:RA0.6.1 WS:RG.0.2 WS:RA0.0.5 FA0.7@1 FB1.5@1 FA0.5@1 FA1.3@1 FB1.1@1 '
        'RA1.0.4 WS:RA0.4.1 WS:RB1.3.5 FB0.3@1 FA1.7@1 FG.2@1 RA1.2.4 WS:RA0.7.5 WS:RA0.3.1 WS:RB1.7.4 FA0.2@1 '
        'WS:RA0.5.5 WS:RG.0.4 FA1.0@1 FB0.1@1 WS:RB1.5.2 FB0.0@1 FA1.2@1 WS:RA1.3.4 FB0.4@1 FB0.7@1 FG.3@1 FG.6@1 '
        'WS:RA1.6.2 FG.1@1 FA1.1@1 WS:RA1.0.4 FG.4@1 FA1.5@1 FG.7@1 FG.5@1 WS:RA1.2.4 FA1.4@1'
    ).split(),
    (
        'LWQ4 LWO4.0 LX2.2 LX2.3 LX2.0 LWQ5 LWO4.2 LXG2 LX2.1 LWO4.3 LWO4.1 LK2.0.1 CO4.0 O.4.0:21 CW4.3 CW4.1 '
        'CW4.2 CW4.0 CX2.2 Q4.2@2 LK2.1.1 Q.4.2:23 CX2.3 Q4.3@2 Q.4.3:21 CX2.0 Q4.0@2 LK2.1.3 Q.4.0:23 CW5.2 '
        'CW5.1 CW5.0 CW5.3 G.6:21 Q5.3@2 LWO5 Q.5.3:21 WS:O.4.0:21 GQ5 CX2.1 LK2.1.2 G.5:23 Q5.1@2 G.7:21 CO4.1 '
        'O.4.1:21 Q.5.1:21 GQ4 WS:Q.4.2:23 HV.6.1:23 LK2.0.2 WS:Q.4.3:21 G.2:23 PK2.0.1 G.5:21 CO4.2 WS:Q.4.0:23 '
        'O.4.2:21 Q5.0@2 WS:G.6:21 Q5.2@2 LK2.0.3 CO4.3 G.3:23 O.4.3:21 PK2.1.1 WS:G.5:23 GL3@2 LK2.0.0 '
        'WS:Q.5.3:21 WS:G.7:21 HK.6.1:23 Q4.1@2 Q.4.1:21 GL2@2 LK2.1.0 WS:HV.6.1:23 WS:G.2:23 HV.6.0:23 '
        'WS:O.4.1:21 PK2.1.3 CO5 AT5.2 AT5.3 WS:Q.5.1:21 WS:G.3:23 HK.6.0:23 G.1:23 PB1@2 G.4:21 WS:G.5:21 '
        'PK2.0.2 PK2.1.2 WS:HK.6.1:23 PA1@2 RB1.5.3 G.0:23 WS:O.4.2:21 PK2.0.3 WS:HV.6.0:23 GL4@2 GL6@2 GL7@2 '
        'WS:O.4.3:21 GM2@2 WS:HK.6.0:23 GM3@2 RA1.7.3 GM6@2 E.2.2:21 GM4@2 E.4.2:21 PK2.0.0 WS:G.1:23 E.6.2:23 '
        'E.3.2:21 RA1.6.3 GM7@2 RB1.0.3 WS:Q.4.1:21 PK2.1.0 WS:G.0:23 E.7.2:23 GL0@2 GL1@2 WS:G.4:21 WS:RB1.5.3 '
        'GM0@2 GM1@2 E.1.2:23 E.0.2:23 AT5.0 WS:RA1.7.3 WS:E.2.2:21 RA1.2.1 PB0@2 WS:E.4.2:21 WS:E.6.2:23 RB0.4.4 '
        'RB0.2.0 RB0.6.4 WS:E.7.2:23 RB0.1.4 WS:E.3.2:21 RB1.7.1 RB0.5.4 RA1.0.1 AT5.1 WS:RA1.6.3 RA1.3.1 '
        'WS:E.1.2:23 RB0.7.1 RB0.0.4 PA0@2 WS:RB1.0.3 WS:E.0.2:23 WS:RA1.2.1 RA0.3.4 RB1.6.4 RA0.1.4 GL5@2 '
        'WS:RB0.4.4 WS:RB0.2.0 WS:RB0.6.4 RB1.1.4 RB1.2.4 WS:RB1.7.1 RB1.4.4 RA0.4.4 WS:RB0.1.4 PG@2 WS:RB0.5.4 '
        'WS:RA1.0.1 RA0.6.4 RG.2.1 RG.4.4 WS:RA1.3.1 WS:RB0.7.1 RG.6.1 RB1.2.2 WS:RB0.0.4 WS:RA0.3.4 RB1.4.2 '
        'RG.1.1 WS:RB1.6.4 RB0.6.2 RG.7.4 RG.3.4 WS:RA0.1.4 WS:RB1.1.4 FB1.2@2 RB1.3.2 RG.5.1 WS:RB1.2.4 '
        'WS:RA0.4.4 FB1.4@2 RG.0.1 WS:RB1.4.4 FB0.6@2 RA1.5.1 RB0.5.2 WS:RA0.6.4 WS:RG.2.1 WS:RG.4.4 FB1.3@2 '
        'RA1.1.4 WS:RB1.2.2 RA0.0.2 WS:RG.6.1 WS:RB1.4.2 FB0.5@2 RB1.6.2 WS:RG.1.1 RA1.4.4 WS:RB0.6.2 WS:RG.7.4 '
        'RA0.7.2 RB0.3.4 RB1.3.4 WS:RG.3.4 WS:RB1.3.2 WS:RG.5.1 WS:RG.0.1 FB1.6@2 RA0.5.2 RA0.2.4 WS:RA1.5.1 '
        'WS:RB0.5.2 RB1.1.2 RA0.0.4 RB0.3.2 WS:RA1.1.4 WS:RA0.0.2 RA0.1.2 FB1.1@2 RA0.2.2 WS:RB1.6.2 WS:RA1.4.4 '
        'FA0.0@2 FB0.3@2 RB0.1.2 RB1.0.5 WS:RA0.7.2 WS:RB0.3.4 RB0.0.2 FA0.1@2 RA0.5.4 WS:RB1.3.4 WS:RA0.5.2 '
        'FA0.2@2 RB0.4.2 WS:RA0.2.4 FB1.0@2 FB0.1@2 RG.3.2 WS:RB1.1.2 RA0.7.4 WS:RB0.3.2 FB0.0@2 FA0.5@2 RA0.6.2 '
        'WS:RA0.0.4 RA1.1.2 WS:RA0.1.2 WS:RA0.2.2 FB0.4@2 FA0.7@2 FG.3@2 RG.4.2 RA0.4.2 RG.7.2 WS:RB0.1.2 '
        'WS:RB1.0.5 FA0.6@2 FA1.1@2 RA0.3.2 RA1.4.2 WS:RB0.0.2 WS:RA0.5.4 WS:RB0.4.2 FG.7@2 WS:RG.3.2 FA0.4@2 '
        'WS:RA0.7.4 FG.4@2 WS:RA1.1.2 FA0.3@2 WS:RA0.6.2 FA1.4@2 WS:RG.4.2 FG.5@2 FB1.7@2 WS:RG.7.2 WS:RA0.4.2 '
        'FG.6@2 FG.0@2 FB0.7@2 WS:RA1.4.2 FB1.5@2 WS:RA0.3.2 FA1.7@2 FA1.3@2 FB0.2@2 FA1.6@2 FG.1@2 FA1.0@2 '
        'FA1.5@2 FG.2@2 FA1.2@2'
    ).split(),
    (
        'LWO7.3 LWQ6 LXG3 LWO7.2 LX3.0 LWQ7 LWO7.0 LWO7.1 LX3.2 LX3.3 LX3.1 CO7.3 O.7.3:30 LK3.0.2 CW6.1 CW6.0 '
        'CW6.2 CW6.3 CO7.2 O.7.2:30 GQ6 LK3.0.1 CX3.0 G.6:32 Q6.0@3 Q.6.0:30 CW7.3 CW7.0 CW7.1 CW7.2 LK3.1.2 GQ7 '
        'G.7:32 CX3.2 CO7.0 Q6.2@3 WS:O.7.3:30 Q.6.2:30 K.5.1.0:32 LK3.1.1 CX3.3 Q6.3@3 CX3.1 WS:G.6:32 Q.6.3:30 '
        'WS:O.7.2:30 V.5.1.1:32 Q6.1@3 LWO6 LK3.1.0 Q.4.2:30 PK3.0.2 WS:Q.6.0:30 WS:G.7:32 V.5.1.0:32 Q7.1@3 '
        'LK3.1.3 QX4@3 WS:Q.6.2:30 K.5.1.1:32 Q.4.0:30 Q.6.1:30 WS:K.5.1.0:32 Q7.2@3 O.7.0:30 Q7.3@3 CO7.1 '
        'Q.7.2:30 LK3.0.0 WS:Q.6.3:30 V.5.0.1:32 Q7.0@3 WS:V.5.1.1:32 PK3.0.1 O.7.1:30 PK3.1.2 LK3.0.3 '
        'WS:Q.4.2:30 V.5.0.0:32 PK3.1.1 WS:V.5.1.0:32 GL2@3 GL4@3 WS:K.5.1.1:32 WS:Q.4.0:30 E.4.3:32 E.2.3:32 '
        'Q.7.0:30 GL3@3 GL5@3 Q.7.1:30 E.3.3:32 WS:Q.6.1:30 K.5.0.1:32 WS:V.5.0.1:32 PK3.1.3 CO6 AW6.3 '
        'WS:O.7.0:30 WS:V.5.0.0:32 K.5.0.0:32 PK3.0.0 WS:E.4.3:32 PA1@3 WS:Q.7.2:30 WS:E.2.3:32 PB1@3 WS:E.3.3:32 '
        'RA1.2.0 RA1.0.0 AW6.1 WS:O.7.1:30 Q.7.3:30 RB1.7.0 RB1.0.0 RB1.5.0 PK3.0.3 PK3.1.0 WS:K.5.0.1:32 PB0@3 '
        'WS:Q.7.0:30 RA1.3.0 RB0.2.3 RA1.6.0 PA0@3 WS:K.5.0.0:32 RA0.1.3 RA1.7.4 RA0.3.3 RA0.4.3 GL0@3 GL6@3 '
        'GL7@3 WS:Q.7.1:30 WS:RA1.2.0 WS:RA1.0.0 GM7@3 E.7.3:30 E.5.3:32 GL1@3 WS:Q.7.3:30 WS:RB1.7.0 WS:RB1.0.0 '
        'RA0.6.3 GM1@3 WS:RA1.3.0 E.1.3:30 WS:RB1.5.0 GM0@3 RB1.2.1 WS:RA0.1.3 E.0.3:30 WS:RB0.2.3 RB0.4.5 '
        'RB1.4.1 RB0.6.1 PG@3 WS:RA1.6.0 WS:RA0.3.3 WS:RA0.4.3 RB0.1.5 RB1.3.1 WS:RA1.7.4 RG.0.0 RB0.5.5 '
        'WS:E.7.3:30 WS:E.5.3:32 FB0.6@3 RB0.7.2 RB0.5.1 WS:RA0.6.3 WS:E.1.3:30 FB0.1@3 FB0.4@3 RB0.0.5 RA0.0.1 '
        'RB0.6.5 RB1.6.1 WS:RB1.2.1 WS:E.0.3:30 WS:RB1.4.1 FB0.5@3 RB1.1.5 WS:RB0.4.5 RA0.7.1 WS:RB0.6.1 RB1.2.5 '
        'WS:RB0.1.5 WS:RB1.3.1 FB1.6@3 RA0.5.1 RB1.6.5 RB1.4.5 RB1.1.1 RB0.3.1 WS:RG.0.0 WS:RB0.5.5 FB1.1@3 '
        'RG.2.2 WS:RB0.7.2 WS:RB0.5.1 WS:RB0.0.5 WS:RA0.0.1 FB1.2@3 FB1.4@3 RG.1.2 RA0.2.1 RB0.1.1 RB0.0.1 RG.4.5 '
        'RB0.4.1 WS:RB0.6.5 FB0.0@3 RG.7.5 WS:RB1.6.1 WS:RB1.1.5 FB1.5@3 RG.5.2 RG.3.5 RG.3.1 WS:RA0.7.1 '
        'WS:RB1.2.5 FB0.7@3 FG.7@3 RA1.5.2 WS:RA0.5.1 WS:RB1.6.5 FG.4@3 RA1.1.1 RG.6.2 WS:RB1.4.5 WS:RB1.1.1 '
        'FG.3@3 RA1.1.5 WS:RB0.3.1 WS:RG.2.2 WS:RG.1.2 FG.1@3 RA1.4.5 WS:RA0.2.1 WS:RG.4.5 FA1.1@3 RB0.3.5 RG.7.1 '
        'FG.5@3 RG.4.1 WS:RG.7.5 RA1.4.1 RG.5.4 WS:RB0.1.1 WS:RB0.0.1 WS:RG.5.2 WS:RG.3.5 FG.6@3 FA1.4@3 FB0.3@3 '
        'RA0.2.5 RG.6.4 RB0.7.4 RA1.7.2 WS:RB0.4.1 WS:RA1.5.2 FB1.3@3 FA1.7@3 RB0.2.5 WS:RG.3.1 WS:RG.6.2 RG.1.4 '
        'WS:RA1.1.1 WS:RA1.1.5 WS:RA1.4.5 WS:RG.7.1 WS:RG.4.1 FA0.2@3 FA1.0@3 FB0.2@3 FA0.0@3 RA1.5.4 RG.2.4 '
        'WS:RB0.3.5 WS:RA1.4.1 FB1.7@3 WS:RG.5.4 WS:RA0.2.5 FA0.1@3 FG.2@3 WS:RG.6.4 FB1.0@3 WS:RB0.7.4 FA1.5@3 '
        'FA0.5@3 WS:RA1.7.2 FA1.2@3 WS:RB0.2.5 FA0.7@3 FA1.3@3 WS:RG.1.4 FA0.6@3 FA1.6@3 WS:RA1.5.4 FG.0@3 '
        'WS:RG.2.4 FA0.4@3 FA0.3@3'
    ).split(),
]


def pallas_dist_sparse_attn_localglobal_htp_kvseq_b2_sq256_skv256_hq4_dh64_kernel(x, Wq, K_ext, V_ext, Wo):
    return make_kernel(CONFIG, PROGRAMS)(x, Wq, K_ext, V_ext, Wo)
```
